```python
import numpy as np

kernel_name = "dist_moe_shared_ep_outshard_n256_d128_e2_h256"

def setup_inputs():
    x = np.random.randn(256, 128).astype(np.float32)
    router_W = np.random.randn(128, 8).astype(np.float32) * 0.1
    scores64 = x.astype(np.float64) @ router_W.astype(np.float64)
    route_idx = np.argsort(-scores64, axis=-1)[:, :1].astype(np.int32)
    expert_W = np.random.randn(8, 128, 256).astype(np.float32) * 0.02
    shared_W = np.random.randn(128, 256).astype(np.float32) * 0.02
    return {"x": x, "router_W": router_W, "route_idx": route_idx, "expert_W": expert_W, "shared_W": shared_W}

def reference(x, router_W, route_idx, expert_W, shared_W):
    scores = x @ router_W
    s_max = scores.max(axis=-1, keepdims=True)
    probs = np.exp(scores - s_max)
    probs = probs / probs.sum(axis=-1, keepdims=True)
    shared = x @ shared_W
    out = np.zeros((256, 256), dtype=np.float32)
    for i in range(256):
        e = int(route_idx[i, 0])
        out[i] = shared[i] + probs[i, e] * (x[i] @ expert_W[e])
    return out
```

```python
import contextlib
import jax
import jax.numpy as jnp
from jax import lax
from jax.experimental import pallas as pl
from jax.experimental.pallas import tpu as pltpu

N_DEV = 4
T = 64
D = 128
H = 256
f32, bf16, u32, i32 = jnp.float32, jnp.bfloat16, jnp.uint32, jnp.int32
MESH = pl.DeviceIdType.MESH


def _pack(y):
    r = lax.bitcast_convert_type(y.astype(bf16).astype(f32), u32)
    return r[:, 128:] | (r[:, :128] >> 16)


def make(order="iaxb", prof=False, two=False, late=True, split=(2, 2), nosem=True, **cp):
  S = (lambda n: jax.named_scope("S_" + n)) if prof else (lambda n: contextlib.nullcontext())
  def kernel(x, router_W, route_idx, expert_W, shared_W):
    def body(x_hbm, rw_hbm, idx_hbm, ew_hbm, sw_hbm, out_ref,
             idx_v, xb, wb, swb, rwb, sbuf, rbuf, send_sem, recv_sem, ld):
        me = lax.axis_index("i")
        odd = me & 1
        dest = [me ^ 2, 1 - odd, 3 - odd, me]

        def load(src, dst, s):
            c = pltpu.make_async_copy(src, dst, ld.at[s])
            c.start()
            return c

        def load_x(k, s):
            return load(x_hbm.at[pl.ds(pl.multiple_of(dest[k] * T, T), T)], xb.at[k], s)

        for ch in order:
            if ch == "i": c_iv = load(idx_hbm, idx_v, 0)
            if ch == "a": c_w0 = load(ew_hbm.at[0], wb.at[0], 1)
            if ch == "x": c_xd = load_x(0, 2)
            if ch == "b": c_w1 = load(ew_hbm.at[1], wb.at[1], 3)
        bar = pltpu.get_barrier_semaphore()
        for k in range(3):
            pl.semaphore_signal(bar, 1, device_id=(dest[k],), device_id_type=MESH)
        def rest():
            return [load_x(1, 4), load_x(2, 5), load_x(3, 6), load(rw_hbm, rwb, 7), load(sw_hbm, swb, 8)]
        if not late: *c_rest, c_sw = rest()

        def row_copy(k, e, g, j):
            return pltpu.make_async_remote_copy(
                sbuf.at[k * 4 + e * 2 + g, pl.ds(j, 1)], rbuf.at[g, pl.ds(j, 1)], send_sem, recv_sem,
                device_id=(dest[k],), device_id_type=MESH)

        sub = lax.broadcasted_iota(i32, (8, 128), 0)
        lane = lax.broadcasted_iota(i32, (8, 128), 1)
        in_group = ((lane >> 5) ^ (odd << 1)) == (sub & 3)
        bit = (jnp.int32(0x8000) >> (lane & 15)).astype(f32)
        w_hi = jnp.where(in_group & ((lane & 16) == 0), bit, 0.0)
        w_lo = jnp.where(in_group & ((lane & 16) != 0), bit, 0.0)
        expert = 2 * me + (sub >> 2)

        with S("idx"):
            c_iv.wait()
        iv = idx_v[...] & 7

        def masks(v):
            hit = v == expert
            hi = jnp.sum(jnp.where(hit, w_hi, 0.0), axis=1, keepdims=True).astype(i32)
            lo = jnp.sum(jnp.where(hit, w_lo, 0.0), axis=1, keepdims=True).astype(i32)
            return (hi << 16) | lo

        m_lo, m_hi = masks(iv[:, :128]), masks(iv[:, 128:])
        src = [(jnp.where(me >= 2, m_lo, m_hi), 0), (m_lo, 2), (m_hi, 2), (jnp.where(me >= 2, m_hi, m_lo), 0)]

        def plan(k):
            m, off = src[k]
            return {(e, g): m[e * 4 + off + g, 0] for e in range(2) for g in range(2)}

        plans = {0: plan(0)}
        if late: *c_rest, c_sw = rest()

        def send(k, e):
            for g in range(2):
                def step(m):
                    nxt = m & (m - 1)
                    row_copy(k, e, g, lax.clz(m ^ nxt)).start()
                    if not (two and k):
                        return nxt
                    nx2 = nxt & (nxt - 1)
                    @pl.when(nxt != 0)
                    def _():
                        row_copy(k, e, g, lax.clz(nxt ^ nx2)).start()
                    return nx2
                lax.while_loop(lambda m: m != 0, step, plans[k][e, g])

        def put(k, e, y):
            for g in range(2):
                sbuf[k * 4 + e * 2 + g] = y[g * 32:(g + 1) * 32]

        def expert_rows(xx, e):
            w = wb[e].astype(bf16)
            if split[e] == 1:
                return _pack(jnp.dot(xx, w, preferred_element_type=f32))
            if split[e] == 2:
                return _pack(jnp.concatenate([jnp.dot(xx[g * 32:(g + 1) * 32], w, preferred_element_type=f32) for g in range(2)], axis=0))
            return _pack(jnp.concatenate([jnp.concatenate(
                [jnp.dot(xx[g * 32:(g + 1) * 32], w[:, h * 128:(h + 1) * 128], preferred_element_type=f32) for h in range(2)], axis=1) for g in range(2)], axis=0))

        c_w0.wait()
        with S("w0x"):
            c_xd.wait()
        xd = xb[0].astype(bf16)
        put(0, 0, expert_rows(xd, 0))
        with S("bar"):
            pl.semaphore_wait(bar, 3)
        send(0, 0)
        with S("w1"):
            c_w1.wait()
        put(0, 1, expert_rows(xd, 1))
        with S("snd01"):
            send(0, 1)

        with S("xr"):
            for c in c_rest: c.wait()
        for k in (1, 2, 3):
            plans[k] = plan(k)
        xm = xb[3].astype(bf16)
        s = lax.dot_general(rwb[...].astype(bf16), xm, (((1,), (1,)), ((), ())), preferred_element_type=f32)
        ex = jnp.exp(s - jnp.max(s, axis=0, keepdims=True))
        half = jnp.where(me >= 2, iv[:, 128:], iv[:, :128])
        mine = jnp.where(odd == 1, half[:, T:], half[:, :T])
        sel = lax.broadcasted_iota(i32, (8, T), 0) == mine
        p = jnp.sum(jnp.where(sel, ex, 0.0), axis=0, keepdims=True) / jnp.sum(ex, axis=0, keepdims=True)
        xr = jnp.concatenate([xb[1].astype(bf16), xb[2].astype(bf16), xm], axis=0)
        for e in range(2):
            y = _pack(jnp.dot(xr, wb[e].astype(bf16), preferred_element_type=f32))
            for k in (1, 2, 3):
                put(k, e, y[(k - 1) * T:k * T])
        for k in (1, 2, 3):
          with S("snd%d" % k):
            for e in range(2):
                send(k, e)
        c_sw.wait()
        shared = jnp.dot(xm, swb[...].astype(bf16), preferred_element_type=f32)
        eye = lax.broadcasted_iota(i32, (T, T), 0) == lax.broadcasted_iota(i32, (T, T), 1)
        pc = jnp.sum(jnp.where(eye, p, 0.0), axis=1, keepdims=True)
        n = jnp.sum(jnp.where((iv >> 1) == me, 1.0, 0.0), axis=1, keepdims=True).astype(i32)[0, 0]

        def drain(c):
            def f(j, carry):
                for _ in range(c):
                    row_copy(0, 0, 0, 0).wait_send()
                return carry
            return f
        with S("drain"):
            lax.fori_loop(0, n >> 3, drain(8), 0)
            lax.fori_loop(0, n & 7, drain(1), 0)
        with S("recv"):
            pltpu.make_async_copy(rbuf, rbuf, recv_sem).wait()
        r = rbuf[...].reshape(T, 128)
        lo = lax.bitcast_convert_type(r << 16, f32)
        hi = lax.bitcast_convert_type(r & jnp.uint32(0xFFFF0000), f32)
        out_ref[:, :128] = shared[:, :128] + pc * lo
        out_ref[:, 128:] = shared[:, 128:] + pc * hi

    hbm = pl.BlockSpec(memory_space=pltpu.HBM)
    return pl.pallas_call(
        body,
        out_shape=jax.ShapeDtypeStruct((T, H), f32),
        in_specs=[hbm] * 5,
        out_specs=pl.BlockSpec(memory_space=pltpu.VMEM),
        scratch_shapes=[
            pltpu.VMEM((1, 256), i32), pltpu.VMEM((4, T, D), f32), pltpu.VMEM((2, D, H), f32),
            pltpu.VMEM((D, H), f32), pltpu.VMEM((8, D), f32),
            pltpu.VMEM((16, 32, 128), u32), pltpu.VMEM((2, 32, 128), u32),
            pltpu.SemaphoreType.DMA, pltpu.SemaphoreType.DMA, pltpu.SemaphoreType.DMA((9,))],
        compiler_params=pltpu.CompilerParams(collective_id=0, disable_semaphore_checks=nosem, **cp),
    )(x, router_W.T, route_idx.reshape(1, 256), expert_W, shared_W)
  return kernel

pallas_dist_moe_shared_ep_outshard_n256_d128_e2_h256_kernel = make()
```

```python
import jax
import jax.numpy as jnp
from jax import lax
from jax.experimental import pallas as pl
from jax.experimental.pallas import tpu as pltpu

N_DEV = 4
N_EXPERTS = 8
LOCAL_EXPERTS = N_EXPERTS // N_DEV
TOKENS = 256
BLOCK = TOKENS // N_DEV
GROUP = 32
GROUPS = BLOCK // GROUP
D = 128
H = 256
LANES = 128

f32, bf16, u32, i32 = jnp.float32, jnp.bfloat16, jnp.uint32, jnp.int32
MESH = pl.DeviceIdType.MESH


def _pack(y):
    bits = lax.bitcast_convert_type(y.astype(bf16).astype(f32), u32)
    return bits[:, LANES:] | (bits[:, :LANES] >> 16)


def _unpack(words):
    return (
        lax.bitcast_convert_type(words << 16, f32),
        lax.bitcast_convert_type(words & jnp.uint32(0xFFFF0000), f32),
    )


def _block_dot(x, w):
    return jnp.concatenate(
        [
            jnp.dot(x[g * GROUP : (g + 1) * GROUP], w, preferred_element_type=f32)
            for g in range(GROUPS)
        ],
        axis=0,
    )


def _body(
    x_hbm,
    router_hbm,
    idx_hbm,
    expert_hbm,
    shared_hbm,
    out_ref,
    idx_buf,
    x_buf,
    expert_buf,
    shared_buf,
    router_buf,
    send_buf,
    recv_buf,
    send_sem,
    recv_sem,
    load_sems,
):
    me = lax.axis_index("i")
    odd = me & 1
    upper = me >= 2
    dest = [me ^ 2, 1 - odd, 3 - odd, me]

    def load(src, dst, sem):
        copy = pltpu.make_async_copy(src, dst, load_sems.at[sem])
        copy.start()
        return copy

    def load_x(k, sem):
        rows = pl.ds(pl.multiple_of(dest[k] * BLOCK, BLOCK), BLOCK)
        return load(x_hbm.at[rows], x_buf.at[k], sem)

    idx_load = load(idx_hbm, idx_buf, 0)
    w0_load = load(expert_hbm.at[0], expert_buf.at[0], 1)
    x_diag_load = load_x(0, 2)
    w1_load = load(expert_hbm.at[1], expert_buf.at[1], 3)

    barrier = pltpu.get_barrier_semaphore()
    for k in range(N_DEV - 1):
        pl.semaphore_signal(barrier, 1, device_id=(dest[k],), device_id_type=MESH)

    sub = lax.broadcasted_iota(i32, (8, LANES), 0)
    lane = lax.broadcasted_iota(i32, (8, LANES), 1)
    in_group = ((lane >> 5) ^ (odd << 1)) == (sub & 3)
    bit = (jnp.int32(0x8000) >> (lane & 15)).astype(f32)
    hi_bit = jnp.where(in_group & ((lane & 16) == 0), bit, 0.0)
    lo_bit = jnp.where(in_group & ((lane & 16) != 0), bit, 0.0)
    expert = LOCAL_EXPERTS * me + (sub >> 2)

    def bitmasks(idx):
        hit = idx == expert
        hi = jnp.sum(jnp.where(hit, hi_bit, 0.0), axis=1, keepdims=True)
        lo = jnp.sum(jnp.where(hit, lo_bit, 0.0), axis=1, keepdims=True)
        return (hi.astype(i32) << 16) | lo.astype(i32)

    idx_load.wait()
    idx = idx_buf[...] & (N_EXPERTS - 1)
    low, high = bitmasks(idx[:, :LANES]), bitmasks(idx[:, LANES:])
    masks = [
        (jnp.where(upper, low, high), 0),
        (low, GROUPS),
        (high, GROUPS),
        (jnp.where(upper, high, low), 0),
    ]

    def words_for(k):
        mask, first = masks[k]
        return [
            [mask[4 * e + first + g, 0] for g in range(GROUPS)]
            for e in range(LOCAL_EXPERTS)
        ]

    def slot(k, e, g):
        return (k * LOCAL_EXPERTS + e) * GROUPS + g

    def stage(k, e, y):
        packed = _pack(y)
        for g in range(GROUPS):
            send_buf[slot(k, e, g)] = packed[g * GROUP : (g + 1) * GROUP]

    def row_copy(k, e, g, j):
        return pltpu.make_async_remote_copy(
            src_ref=send_buf.at[slot(k, e, g), pl.ds(j, 1)],
            dst_ref=recv_buf.at[g, pl.ds(j, 1)],
            send_sem=send_sem,
            recv_sem=recv_sem,
            device_id=(dest[k],),
            device_id_type=MESH,
        )

    def send(k, e, words):
        for g in range(GROUPS):

            def send_lowest_bit(word, g=g):
                rest = word & (word - 1)
                row_copy(k, e, g, lax.clz(word ^ rest)).start()
                return rest

            lax.while_loop(lambda word: word != 0, send_lowest_bit, words[e][g])

    diag_words = words_for(0)
    rest_loads = [load_x(k, 3 + k) for k in range(1, N_DEV)]
    rest_loads.append(load(router_hbm, router_buf, 7))
    shared_load = load(shared_hbm, shared_buf, 8)

    w0_load.wait()
    x_diag_load.wait()
    x_diag = x_buf[0].astype(bf16)
    stage(0, 0, _block_dot(x_diag, expert_buf[0].astype(bf16)))
    pl.semaphore_wait(barrier, N_DEV - 1)
    send(0, 0, diag_words)
    w1_load.wait()
    stage(0, 1, _block_dot(x_diag, expert_buf[1].astype(bf16)))
    send(0, 1, diag_words)

    for copy in rest_loads:
        copy.wait()
    rest_words = {k: words_for(k) for k in range(1, N_DEV)}
    hosted = jnp.where((idx >> 1) == me, 1.0, 0.0)
    n_sent = jnp.sum(hosted, axis=1, keepdims=True).astype(i32)[0, 0]

    x_mine = x_buf[N_DEV - 1].astype(bf16)
    scores = lax.dot_general(
        router_buf[...].astype(bf16),
        x_mine,
        (((1,), (1,)), ((), ())),
        preferred_element_type=f32,
    )
    weights = jnp.exp(scores - jnp.max(scores, axis=0, keepdims=True))
    my_half = jnp.where(upper, idx[:, LANES:], idx[:, :LANES])
    my_idx = jnp.where(odd == 1, my_half[:, BLOCK:], my_half[:, :BLOCK])
    chosen = lax.broadcasted_iota(i32, (N_EXPERTS, BLOCK), 0) == my_idx
    prob = jnp.sum(
        jnp.where(chosen, weights, 0.0), axis=0, keepdims=True
    ) / jnp.sum(weights, axis=0, keepdims=True)

    x_rest = jnp.concatenate(
        [x_buf[1].astype(bf16), x_buf[2].astype(bf16), x_mine], axis=0
    )
    for e in range(LOCAL_EXPERTS):
        y = jnp.dot(x_rest, expert_buf[e].astype(bf16), preferred_element_type=f32)
        for k in range(1, N_DEV):
            stage(k, e, y[(k - 1) * BLOCK : k * BLOCK])
    for k in range(1, N_DEV):
        for e in range(LOCAL_EXPERTS):
            send(k, e, rest_words[k])

    shared_load.wait()
    shared = _block_dot(x_mine, shared_buf[...].astype(bf16))
    eye = lax.broadcasted_iota(i32, (BLOCK, BLOCK), 0) == lax.broadcasted_iota(
        i32, (BLOCK, BLOCK), 1
    )
    prob = jnp.sum(jnp.where(eye, prob, 0.0), axis=1, keepdims=True)

    def wait_sends(count):
        def step(_, carry):
            for _ in range(count):
                row_copy(0, 0, 0, 0).wait_send()
            return carry

        return step

    lax.fori_loop(0, n_sent >> 3, wait_sends(8), 0)
    lax.fori_loop(0, n_sent & 7, wait_sends(1), 0)

    pltpu.make_async_copy(recv_buf, recv_buf, recv_sem).wait()
    left, right = _unpack(recv_buf[...].reshape(BLOCK, LANES))
    out_ref[:, :LANES] = shared[:, :LANES] + prob * left
    out_ref[:, LANES:] = shared[:, LANES:] + prob * right


def pallas_dist_moe_shared_ep_outshard_n256_d128_e2_h256_kernel(
    x: jax.Array,
    router_W: jax.Array,
    route_idx: jax.Array,
    expert_W: jax.Array,
    shared_W: jax.Array,
):
    return pl.pallas_call(
        _body,
        out_shape=jax.ShapeDtypeStruct((BLOCK, H), f32),
        in_specs=[pl.BlockSpec(memory_space=pltpu.HBM)] * 5,
        out_specs=pl.BlockSpec(memory_space=pltpu.VMEM),
        scratch_shapes=[
            pltpu.VMEM((1, TOKENS), i32),
            pltpu.VMEM((N_DEV, BLOCK, D), f32),
            pltpu.VMEM((LOCAL_EXPERTS, D, H), f32),
            pltpu.VMEM((D, H), f32),
            pltpu.VMEM((N_EXPERTS, D), f32),
            pltpu.VMEM((N_DEV * LOCAL_EXPERTS * GROUPS, GROUP, LANES), u32),
            pltpu.VMEM((GROUPS, GROUP, LANES), u32),
            pltpu.SemaphoreType.DMA,
            pltpu.SemaphoreType.DMA,
            pltpu.SemaphoreType.DMA((9,)),
        ],
        compiler_params=pltpu.CompilerParams(
            collective_id=0, disable_semaphore_checks=True
        ),
    )(
        x,
        router_W.T,
        route_idx.reshape(1, TOKENS),
        expert_W,
        shared_W,
    )
```
